```python
import numpy as np

kernel_name = "dist_moe_cap_ep_outshard_n2048_d512_e8_h1024"

def setup_inputs():
    x = np.random.randn(2048, 512).astype(np.float32)
    router_W = np.random.randn(512, 32).astype(np.float32) * 0.1
    scores64 = x.astype(np.float64) @ router_W.astype(np.float64)
    route_idx = np.argsort(-scores64, axis=-1)[:, :1].astype(np.int32)
    expert_W = np.random.randn(32, 512, 1024).astype(np.float32) * 0.02
    return {"x": x, "router_W": router_W, "route_idx": route_idx, "expert_W": expert_W}

def reference(x, router_W, route_idx, expert_W):
    counts = np.zeros(32, dtype=np.int64)
    out = np.zeros((2048, 1024), dtype=np.float32)
    for i in range(2048):
        e = int(route_idx[i, 0])
        if counts[e] < 51:
            out[i] = x[i] @ expert_W[e]
            counts[e] += 1
    return out
```

```python
import jax
import jax.numpy as jnp
from jax import lax
from jax.experimental import pallas as pl
from jax.experimental.pallas import tpu as pltpu

N_TOK = 2048
D_IN = 512
D_OUT = 1024
HALF = D_OUT // 2
N_DEV = 4
N_EXP = 32
E_LOC = N_EXP // N_DEV
CAP = 51
SLOTS = 64
ROWS = N_TOK // N_DEV
BLK = 256


def _body(x_hbm, r_ref, w_hbm, out_hbm,
          w_vmem, xg, ysend, stage, outbuf, zrow,
          tok_v, keep_v, tok_s, keep_s,
          w_sems, g_sems, m_sems, send_sem, recv_sem, o_sem):
    me = lax.axis_index("i")

    def w_copy(e):
        return pltpu.make_async_copy(w_hbm.at[e], w_vmem.at[e], w_sems.at[e])

    w_copy(0).start()
    w_copy(1).start()

    r = r_ref[...]
    e_iota = lax.broadcasted_iota(jnp.int32, (N_EXP, N_TOK), 0)
    onehot = (r == e_iota)
    oh_f = onehot.astype(jnp.float32)
    oh_b = oh_f.astype(jnp.bfloat16)
    jj = lax.broadcasted_iota(jnp.int32, (BLK, BLK), 0)
    ii = lax.broadcasted_iota(jnp.int32, (BLK, BLK), 1)
    upper = (jj < ii).astype(jnp.float32).astype(jnp.bfloat16)
    carry = jnp.zeros((N_EXP, 1), jnp.float32)
    pos_parts = []
    for b in range(N_TOK // BLK):
        ob = oh_b[:, b * BLK:(b + 1) * BLK]
        of = oh_f[:, b * BLK:(b + 1) * BLK]
        c = jnp.dot(ob, upper, preferred_element_type=jnp.float32) + carry
        pos_parts.append(jnp.sum(of * c, axis=0, keepdims=True))
        carry = carry + jnp.sum(of, axis=1, keepdims=True)
    pos = jnp.concatenate(pos_parts, axis=1).astype(jnp.int32)
    keep = pos < CAP

    tok_i = lax.broadcasted_iota(jnp.int32, (1, N_TOK), 1)
    le = r - me * E_LOC
    row = lax.broadcasted_iota(jnp.int32, (3 * E_LOC, N_TOK), 0)
    sel = jnp.logical_and(keep, (row % E_LOC) == le)
    val = jnp.where(row < E_LOC, tok_i >> 6,
                    jnp.where(row < 2 * E_LOC, tok_i & 63, 1))
    a_mat = jnp.where(sel, val, 0).astype(jnp.float32).astype(jnp.bfloat16)
    s_iota = lax.broadcasted_iota(jnp.int32, (128, N_TOK), 0)
    b_mat = (pos == s_iota).astype(jnp.float32).astype(jnp.bfloat16)
    t = lax.dot_general(a_mat, b_mat, (((1,), (1,)), ((), ())),
                        preferred_element_type=jnp.float32)
    ti = t.astype(jnp.int32)
    tok = ti[0:E_LOC] * 64 + ti[E_LOC:2 * E_LOC]
    tok = jnp.where(ti[2 * E_LOC:3 * E_LOC] > 0, tok, -1)
    tok_v[...] = tok
    keep_v[...] = keep.astype(jnp.int32)
    c1 = pltpu.make_async_copy(tok_v, tok_s, m_sems.at[0])
    c2 = pltpu.make_async_copy(keep_v, keep_s, m_sems.at[1])
    c1.start()
    c2.start()
    xg[...] = jnp.zeros(xg.shape, xg.dtype)
    zrow[...] = jnp.zeros(zrow.shape, zrow.dtype)
    c1.wait()

    for e in range(E_LOC):
        def g_body(s, _, e=e):
            tkn = jnp.maximum(tok_s[e, s], 0)
            pltpu.make_async_copy(x_hbm.at[pl.ds(tkn, 1)], xg.at[e, pl.ds(s, 1)],
                                  g_sems.at[e]).start()
            return 0
        lax.fori_loop(0, CAP, g_body, 0)

    c2.wait()

    def z_copy(rr):
        return pltpu.make_async_remote_copy(
            src_ref=zrow.at[pl.ds(0, 1)], dst_ref=stage.at[pl.ds(rr, 1)],
            send_sem=send_sem, recv_sem=recv_sem,
            device_id=(me,), device_id_type=pl.DeviceIdType.MESH)

    def z_body(rr, n):
        dropped = keep_s[0, me * ROWS + rr] == 0

        @pl.when(dropped)
        def _():
            z_copy(rr).start()
        return n + dropped.astype(jnp.int32)
    n_sent = lax.fori_loop(0, ROWS, z_body, 0)

    for e in range(E_LOC):
        w_copy(e).wait()
        if e + 2 < E_LOC:
            w_copy(e + 2).start()
        pltpu.make_async_copy(xg.at[e, pl.ds(0, 48)], xg.at[e, pl.ds(0, 48)],
                              g_sems.at[e]).wait()
        for s in range(48, CAP):
            pltpu.make_async_copy(xg.at[e, pl.ds(s, 1)], xg.at[e, pl.ds(s, 1)],
                                  g_sems.at[e]).wait()
        xe = xg[e].astype(jnp.bfloat16)
        we = w_vmem[e].astype(jnp.bfloat16)
        y = jnp.dot(xe, we, preferred_element_type=jnp.float32)
        yb = y.astype(jnp.bfloat16).astype(jnp.float32)
        u = pltpu.bitcast(yb, jnp.uint32)
        ysend[e] = (u[:, HALF:] & jnp.uint32(0xFFFF0000)) | (u[:, :HALF] >> 16)

        def s_body(s, n, e=e):
            tkn = tok_s[e, s]
            valid = tkn >= 0

            @pl.when(valid)
            def _():
                pltpu.make_async_remote_copy(
                    src_ref=ysend.at[e, pl.ds(s, 1)],
                    dst_ref=stage.at[pl.ds(tkn & (ROWS - 1), 1)],
                    send_sem=send_sem, recv_sem=recv_sem,
                    device_id=(tkn >> 9,), device_id_type=pl.DeviceIdType.MESH).start()
            return n + valid.astype(jnp.int32)
        n_sent = lax.fori_loop(0, CAP, s_body, n_sent)

    pltpu.make_async_copy(stage, stage, recv_sem).wait()
    w = stage[...]
    outbuf[:, :HALF] = pltpu.bitcast(w << 16, jnp.float32)
    outbuf[:, HALF:] = pltpu.bitcast(w & jnp.uint32(0xFFFF0000), jnp.float32)
    oc = pltpu.make_async_copy(outbuf, out_hbm, o_sem)
    oc.start()

    def ws_body(_, c):
        z_copy(0).wait_send()
        return c
    lax.fori_loop(0, n_sent, ws_body, 0)
    oc.wait()


def pallas_dist_moe_cap_ep_outshard_n2048_d512_e8_h1024_kernel(
    x: jax.Array,
    router_W: jax.Array,
    route_idx: jax.Array,
    expert_W: jax.Array,
):
    del router_W
    r_row = route_idx.reshape(1, N_TOK).astype(jnp.int32)
    return pl.pallas_call(
        _body,
        out_shape=jax.ShapeDtypeStruct((ROWS, D_OUT), jnp.float32),
        in_specs=[
            pl.BlockSpec(memory_space=pl.ANY),
            pl.BlockSpec(memory_space=pltpu.VMEM),
            pl.BlockSpec(memory_space=pl.ANY),
        ],
        out_specs=pl.BlockSpec(memory_space=pl.ANY),
        scratch_shapes=[
            pltpu.VMEM((E_LOC, D_IN, D_OUT), jnp.float32),
            pltpu.VMEM((E_LOC, SLOTS, D_IN), jnp.float32),
            pltpu.VMEM((E_LOC, SLOTS, HALF), jnp.uint32),
            pltpu.VMEM((ROWS, HALF), jnp.uint32),
            pltpu.VMEM((ROWS, D_OUT), jnp.float32),
            pltpu.VMEM((8, HALF), jnp.uint32),
            pltpu.VMEM((E_LOC, 128), jnp.int32),
            pltpu.VMEM((1, N_TOK), jnp.int32),
            pltpu.SMEM((E_LOC, 128), jnp.int32),
            pltpu.SMEM((1, N_TOK), jnp.int32),
            pltpu.SemaphoreType.DMA((E_LOC,)),
            pltpu.SemaphoreType.DMA((E_LOC,)),
            pltpu.SemaphoreType.DMA((2,)),
            pltpu.SemaphoreType.DMA,
            pltpu.SemaphoreType.DMA,
            pltpu.SemaphoreType.DMA,
        ],
        compiler_params=pltpu.CompilerParams(
            vmem_limit_bytes=64 * 1024 * 1024,
        ),
    )(x, r_row, expert_W)
```

```python
import jax
import jax.numpy as jnp
from jax import lax
from jax.experimental import pallas as pl
from jax.experimental.pallas import tpu as pltpu

N_TOK = 2048
D_IN = 512
D_OUT = 1024
HALF = D_OUT // 2
N_DEV = 4
N_EXP = 32
E_LOC = N_EXP // N_DEV
CAP = 51
GSLOTS = 56
SLOTS = 64
ROWS = N_TOK // N_DEV
BLK = 256
NG = D_OUT // 256
LAST_PIECES = ((0, 1), (2,), (3,))

A_SIZES = (2048, 2048, 1024, 512, 256, 128, 64, 32, 16, 8)
B_SIZES = (128, 128, 64, 32, 16, 8)
A_TOTAL = 2 * ROWS * NG
B_TOTAL = 256


def _filler_copies(n, sizes, src, dst, sem):
    off = 0
    for size in sizes:
        take = n >= size

        @pl.when(take)
        def _(off=off, size=size):
            pltpu.make_async_copy(src.at[pl.ds(0, size)], dst.at[pl.ds(off, size)], sem).start()
        n = n - jnp.where(take, size, 0)
        off += size
    for k in range(7):
        @pl.when(n > k)
        def _(k=k, off=off):
            pltpu.make_async_copy(src.at[pl.ds(k, 1)], dst.at[pl.ds(off + k, 1)], sem).start()


def _body(x_hbm, r_hbm, w_hbm, out_hbm,
          r_ref, w_vmem, xg, ysend, stage, outbuf, fill_src, fill_a, fill_b,
          tok_v, tok_s,
          w_sems, wl_sems, g_sems, m_sem, o_sems, send_sem, recv_a, recv_b):
    me = lax.axis_index("i")
    last = E_LOC - 1

    def w_copy(e):
        return pltpu.make_async_copy(w_hbm.at[e], w_vmem.at[e], w_sems.at[e])

    def wl_copy(k):
        gs = LAST_PIECES[k]
        cols = pl.ds(gs[0] * 256, 256 * len(gs))
        return pltpu.make_async_copy(w_hbm.at[last, :, cols], w_vmem.at[last, :, cols],
                                     wl_sems.at[k])

    rc = pltpu.make_async_copy(r_hbm, r_ref, m_sem)
    rc.start()
    for e in range(last):
        w_copy(e).start(priority=1)
    for k in range(len(LAST_PIECES)):
        wl_copy(k).start(priority=1)
    stage[...] = jnp.zeros(stage.shape, stage.dtype)
    barrier = pltpu.get_barrier_semaphore()
    for k in range(1, N_DEV):
        pl.semaphore_signal(barrier, inc=1, device_id=((me + k) % N_DEV,),
                            device_id_type=pl.DeviceIdType.MESH)
    rc.wait()

    r = r_ref[...]
    e_iota = lax.broadcasted_iota(jnp.int32, (N_EXP, N_TOK), 0)
    oh_f = (r == e_iota).astype(jnp.float32)
    oh_b = oh_f.astype(jnp.bfloat16)
    jj = lax.broadcasted_iota(jnp.int32, (BLK, BLK), 0)
    ii = lax.broadcasted_iota(jnp.int32, (BLK, BLK), 1)
    upper = (jj < ii).astype(jnp.float32).astype(jnp.bfloat16)
    carry = jnp.zeros((N_EXP, 1), jnp.float32)
    pos_parts = []
    for b in range(N_TOK // BLK):
        ob = oh_b[:, b * BLK:(b + 1) * BLK]
        of = oh_f[:, b * BLK:(b + 1) * BLK]
        c = jnp.dot(ob, upper, preferred_element_type=jnp.float32) + carry
        pos_parts.append(jnp.sum(of * c, axis=0, keepdims=True))
        carry = carry + jnp.sum(of, axis=1, keepdims=True)
    pos = jnp.concatenate(pos_parts, axis=1).astype(jnp.int32)
    keep = pos < CAP

    tok_i = lax.broadcasted_iota(jnp.int32, (1, N_TOK), 1)
    le = r - me * E_LOC
    row = lax.broadcasted_iota(jnp.int32, (3 * E_LOC, N_TOK), 0)
    sel = jnp.logical_and(keep, (row % E_LOC) == le)
    val = jnp.where(row < E_LOC, tok_i >> 6,
                    jnp.where(row < 2 * E_LOC, tok_i & 63, 1))
    a_mat = jnp.where(sel, val, 0).astype(jnp.float32).astype(jnp.bfloat16)
    s_iota = lax.broadcasted_iota(jnp.int32, (128, N_TOK), 0)
    b_mat = (pos == s_iota).astype(jnp.float32).astype(jnp.bfloat16)
    t = lax.dot_general(a_mat, b_mat, (((1,), (1,)), ((), ())),
                        preferred_element_type=jnp.float32)
    ti = t.astype(jnp.int32)
    filled = ti[2 * E_LOC:3 * E_LOC] > 0
    tok = ti[0:E_LOC] * 64 + ti[E_LOC:2 * E_LOC]
    lane = lax.broadcasted_iota(jnp.int32, (E_LOC, 128), 1)
    srow = lax.broadcasted_iota(jnp.int32, (E_LOC, 128), 0)
    dst_dev = jnp.where(filled, tok >> 9, me)
    dst_row = jnp.where(filled, tok & (ROWS - 1), ROWS + srow * SLOTS + lane)
    fill_e = jnp.sum(filled.astype(jnp.int32), axis=1, keepdims=True)
    n_fill = jnp.sum(fill_e, axis=0, keepdims=True)
    n_fill_l = fill_e[last:last + 1]
    mine = jnp.logical_and(keep, (tok_i >> 9) == me)
    n_keep = jnp.sum(mine.astype(jnp.int32), axis=1, keepdims=True)
    mine_l = jnp.logical_and(mine, (r & (E_LOC - 1)) == last)
    n_keep_l = jnp.sum(mine_l.astype(jnp.int32), axis=1, keepdims=True)
    n_b = n_keep_l + (CAP - n_fill_l)
    n_a = NG * (n_keep + (E_LOC * CAP - n_fill)) - n_b
    tok = jnp.where(jnp.logical_and(srow == 0, lane == 127), A_TOTAL - n_a, tok)
    tok = jnp.where(jnp.logical_and(srow == 0, lane == 126), B_TOTAL - n_b, tok)
    tok_v[0] = tok
    tok_v[1] = dst_dev
    tok_v[2] = dst_row
    mc = pltpu.make_async_copy(tok_v, tok_s, m_sem)
    mc.start()
    xg[...] = jnp.zeros(xg.shape, xg.dtype)
    fill_src[...] = jnp.zeros(fill_src.shape, fill_src.dtype)
    mc.wait()

    def gather(e):
        for s in range(GSLOTS):
            pltpu.make_async_copy(x_hbm.at[pl.ds(tok_s[0, e, s], 1)], xg.at[e, pl.ds(s, 1)],
                                  g_sems.at[e]).start()

    def gather_wait(e):
        rows = xg.at[e, pl.ds(0, GSLOTS)]
        pltpu.make_async_copy(rows, rows, g_sems.at[e]).wait()

    def pack(y):
        u = pltpu.bitcast(y.astype(jnp.bfloat16).astype(jnp.float32), jnp.uint32)
        parts = []
        for g in range(y.shape[1] // 256):
            lo = u[:, g * 256:g * 256 + 128]
            hi = u[:, g * 256 + 128:g * 256 + 256]
            parts.append((hi & jnp.uint32(0xFFFF0000)) | (lo >> 16))
        return parts[0] if len(parts) == 1 else jnp.concatenate(parts, axis=1)

    def send(e, w0, nw, recv_sem):
        for s in range(CAP):
            pltpu.make_async_remote_copy(
                src_ref=ysend.at[e, pl.ds(s, 1), pl.ds(w0, nw)],
                dst_ref=stage.at[pl.ds(tok_s[2, e, s], 1), pl.ds(w0, nw)],
                send_sem=send_sem, recv_sem=recv_sem,
                device_id=(tok_s[1, e, s],), device_id_type=pl.DeviceIdType.MESH).start()

    gather(0)
    gather(1)
    _filler_copies(tok_s[0, 0, 127], A_SIZES, fill_src, fill_a, recv_a)
    _filler_copies(tok_s[0, 0, 126], B_SIZES, fill_src, fill_b, recv_b)
    pl.semaphore_wait(barrier, N_DEV - 1)

    for e in range(last):
        w_copy(e).wait()
        gather_wait(e)
        xe = xg[e].astype(jnp.bfloat16)
        we = w_vmem[e].astype(jnp.bfloat16)
        ysend[e] = pack(jnp.dot(xe, we, preferred_element_type=jnp.float32))
        send(e, 0, HALF, recv_a)
        if e + 2 < E_LOC:
            gather(e + 2)

    gather_wait(last)
    xe = xg[last].astype(jnp.bfloat16)
    for k, gs in enumerate(LAST_PIECES):
        g0, n = gs[0], len(gs)
        wl_copy(k).wait()
        wk = w_vmem[last, :, g0 * 256:(g0 + n) * 256].astype(jnp.bfloat16)
        ysend[last, :, g0 * 128:(g0 + n) * 128] = pack(
            jnp.dot(xe, wk, preferred_element_type=jnp.float32))
        send(last, g0 * 128, n * 128, recv_b if gs[-1] == NG - 1 else recv_a)

    def out_copy(g):
        cols = pl.ds(g * 256, 256)
        return pltpu.make_async_copy(outbuf.at[:, cols], out_hbm.at[:, cols], o_sems.at[g])

    def unpack(g):
        w = stage[0:ROWS, g * 128:(g + 1) * 128]
        outbuf[:, g * 256:g * 256 + 128] = pltpu.bitcast(w << 16, jnp.float32)
        outbuf[:, g * 256 + 128:g * 256 + 256] = pltpu.bitcast(
            w & jnp.uint32(0xFFFF0000), jnp.float32)
        out_copy(g).start()

    pltpu.make_async_copy(stage, stage, recv_a).wait()
    for g in range(NG - 1):
        unpack(g)
    tb = fill_b.at[pl.ds(0, B_TOTAL)]
    pltpu.make_async_copy(tb, tb, recv_b).wait()
    unpack(NG - 1)
    sent = fill_a.at[pl.ds(0, E_LOC * CAP * NG)]
    pltpu.make_async_copy(sent, sent, send_sem).wait()
    for g in range(NG):
        out_copy(g).wait()


def pallas_dist_moe_cap_ep_outshard_n2048_d512_e8_h1024_kernel(
    x: jax.Array,
    router_W: jax.Array,
    route_idx: jax.Array,
    expert_W: jax.Array,
):
    del router_W
    r_row = route_idx.reshape(1, N_TOK).astype(jnp.int32)
    return pl.pallas_call(
        _body,
        out_shape=jax.ShapeDtypeStruct((ROWS, D_OUT), jnp.float32),
        in_specs=[
            pl.BlockSpec(memory_space=pl.ANY),
            pl.BlockSpec(memory_space=pl.ANY),
            pl.BlockSpec(memory_space=pl.ANY),
        ],
        out_specs=pl.BlockSpec(memory_space=pl.ANY),
        scratch_shapes=[
            pltpu.VMEM((1, N_TOK), jnp.int32),
            pltpu.VMEM((E_LOC, D_IN, D_OUT), jnp.float32),
            pltpu.VMEM((E_LOC, SLOTS, D_IN), jnp.float32),
            pltpu.VMEM((E_LOC, SLOTS, HALF), jnp.uint32),
            pltpu.VMEM((2 * ROWS, HALF), jnp.uint32),
            pltpu.VMEM((ROWS, D_OUT), jnp.float32),
            pltpu.VMEM((2048, 128), jnp.uint32),
            pltpu.VMEM((sum(A_SIZES) + 8, 128), jnp.uint32),
            pltpu.VMEM((sum(B_SIZES) + 8, 128), jnp.uint32),
            pltpu.VMEM((3, E_LOC, 128), jnp.int32),
            pltpu.SMEM((3, E_LOC, 128), jnp.int32),
            pltpu.SemaphoreType.DMA((E_LOC - 1,)),
            pltpu.SemaphoreType.DMA((len(LAST_PIECES),)),
            pltpu.SemaphoreType.DMA((E_LOC,)),
            pltpu.SemaphoreType.DMA,
            pltpu.SemaphoreType.DMA((NG,)),
            pltpu.SemaphoreType.DMA,
            pltpu.SemaphoreType.DMA,
            pltpu.SemaphoreType.DMA,
        ],
        compiler_params=pltpu.CompilerParams(
            vmem_limit_bytes=64 * 1024 * 1024,
            collective_id=0,
        ),
    )(x, r_row, expert_W)
```
